```python
import numpy as np

kernel_name = "dist_sort_i_m128_n64"

def setup_inputs():
    return {"x": np.random.randn(512, 64).astype(np.float32)}

def reference(x: np.ndarray) -> np.ndarray:
    return np.sort(x, axis=0)
```

```python
import jax
import jax.numpy as jnp
from jax import lax
from jax.experimental import pallas as pl
from jax.experimental.pallas import tpu as pltpu

F32 = jnp.float32
BF16 = jnp.bfloat16
MESH = pl.DeviceIdType.MESH

SORT16 = (
    ((0, 13), (1, 12), (2, 15), (3, 14), (4, 8), (5, 6), (7, 11), (9, 10)),
    ((0, 5), (1, 7), (2, 9), (3, 4), (6, 13), (8, 14), (10, 15), (11, 12)),
    ((0, 1), (2, 3), (4, 5), (6, 8), (7, 9), (10, 11), (12, 13), (14, 15)),
    ((0, 2), (1, 3), (4, 10), (5, 11), (6, 7), (8, 9), (12, 14), (13, 15)),
    ((1, 2), (3, 12), (4, 6), (5, 7), (8, 10), (9, 11), (13, 14)),
    ((1, 4), (2, 6), (5, 8), (7, 10), (9, 13), (11, 14)),
    ((2, 4), (3, 6), (9, 12), (11, 13)),
    ((3, 5), (6, 8), (7, 9), (10, 12)),
    ((3, 4), (5, 6), (7, 8), (9, 10), (11, 12)),
    ((6, 7), (8, 9)),
)
TREE16 = ((((((0, 2), (4, 5)), ((1, 3), (6, 7))), ((8, 9), (10, 11))), ((12, 13), 14)), 15)
RUN_VBITS = (0, 4, 5, 6)


def _sperm(x, idx):
    return jnp.take_along_axis(x, idx, axis=0, mode="promise_in_bounds")


def _insert(s, p):
    lo = [jnp.minimum(e, p) for e in s]
    return [lo[0]] + [jnp.maximum(s[i - 1], lo[i]) for i in range(1, len(s))] + [jnp.maximum(s[-1], p)]


def _odd_even_merge(a, b):
    if not a or not b:
        return list(a) + list(b)
    if len(b) == 1:
        return _insert(a, b[0])
    if len(a) == 1:
        return _insert(b, a[0])
    ev = _odd_even_merge(a[0::2], b[0::2])
    od = _odd_even_merge(a[1::2], b[1::2])
    out = [ev[0]]
    i = 0
    while i < len(od) and i + 1 < len(ev):
        out += [jnp.minimum(od[i], ev[i + 1]), jnp.maximum(od[i], ev[i + 1])]
        i += 1
    return out + od[i:] + ev[i + 1:]


def _tree_sort(vs, t):
    if isinstance(t, int):
        return [vs[t]]
    return _odd_even_merge(_tree_sort(vs, t[0]), _tree_sort(vs, t[1]))


def _clean(vs, lay, bits, evict, sub):
    vs, lay = list(vs), dict(lay)
    for b in bits:
        kind, p = lay[b]
        if kind == "v":
            for v in range(len(vs)):
                if not (v >> p) & 1:
                    x, y = vs[v], vs[v | (1 << p)]
                    vs[v], vs[v | (1 << p)] = jnp.minimum(x, y), jnp.maximum(x, y)
        else:
            e = evict[b]
            ep = lay[e][1]
            m = (sub & (1 << p)) != 0
            idx = sub ^ (1 << p)
            for v in range(len(vs)):
                if not (v >> ep) & 1:
                    x, y = vs[v], vs[v | (1 << ep)]
                    u = jnp.where(m, y, x)
                    t = _sperm(jnp.where(m, x, y), idx)
                    vs[v], vs[v | (1 << ep)] = jnp.minimum(u, t), jnp.maximum(u, t)
            lay[b], lay[e] = ("v", ep), ("s", p)
    return vs, lay


def _canon(vs, lay, vbits):
    out = [vs[sum(((v >> k) & 1) << lay[b][1] for k, b in enumerate(vbits))] for v in range(len(vs))]
    lay = dict(lay)
    for k, b in enumerate(vbits):
        lay[b] = ("v", k)
    return out, lay


def _sort128(vs, sub, tree=None):
    vs = list(vs)
    if tree is not None:
        vs = _tree_sort(vs, tree)
    else:
        for layer in SORT16:
            for a, b in layer:
                vs[a], vs[b] = jnp.minimum(vs[a], vs[b]), jnp.maximum(vs[a], vs[b])
    lay = {0: ("v", 0), 1: ("v", 1), 2: ("v", 2), 3: ("v", 3), 4: ("s", 2), 5: ("s", 1), 6: ("s", 0)}
    for t in (4, 5, 6):
        idx = sub ^ sum(1 << lay[b][1] for b in range(t + 1) if lay[b][0] == "s")
        pe = lay[0][1]
        ws = list(vs)
        for v in range(16):
            if not (v >> pe) & 1:
                x, y = vs[v], _sperm(vs[v ^ 15], idx)
                ws[v], ws[v | (1 << pe)] = jnp.minimum(x, y), jnp.maximum(x, y)
        lay[0], lay[t] = lay[t], lay[0]
        vs, lay = _clean(ws, lay, range(t - 1, -1, -1), {b: b + 1 for b in range(7)}, sub)
    return _canon(vs, lay, RUN_VBITS)


def _move_bits(val, src, dst):
    if list(src) == list(dst):
        return val
    out = None
    for sp, dp in zip(src, dst):
        t = val & (1 << sp)
        t = t << (dp - sp) if dp >= sp else t >> (sp - dp)
        out = t if out is None else out | t
    return out


def _mirror(vs, lay, dlay, sub):
    vb = sorted((b for b in dlay if dlay[b][0] == "v"), key=lambda b: dlay[b][1])
    vs, lay = _canon(vs, lay, vb)
    sb = [b for b in dlay if dlay[b][0] == "s"]
    idx = _move_bits(sub ^ 7, [dlay[b][1] for b in sb], [lay[b][1] for b in sb])
    return [_sperm(vs[v ^ (len(vs) - 1)], idx) for v in range(len(vs))]


def _skew_roll(xs, sub, lane):
    us = list(xs)
    for b in range(3):
        m = (lane & (1 << b)) != 0
        us = [jnp.where(m, us[(v + (1 << b)) % 8], us[v]) for v in range(8)]
    ys = [_sperm(us[v], (sub + ((lane + v) >> 3)) & 7) for v in range(8)]
    r1 = [pltpu.roll(ys[v], v, 1, stride=8, stride_axis=0) for v in range(8)]
    r2 = [pltpu.roll(ys[v], v + 64, 1, stride=8, stride_axis=0) for v in range(8)]
    return r1, r2


def _to_lanes(xs, sub, lane):
    r1, r2 = _skew_roll(xs, sub, lane)
    return r1 + r2


def _from_lanes(vs, lay, sub, lane, lane_mod64):
    vs, lay = _canon(vs, lay, (0, 1, 2))
    assert [lay[b] for b in (3, 4, 5)] == [("s", 0), ("s", 1), ("s", 2)]
    r1, r2 = _skew_roll(vs, sub, lane)
    wrap = lane_mod64 - 8 * sub
    ws = [_sperm(jnp.where(wrap < v, r2[v], r1[v]), (((lane - v) >> 3) - sub) & 7) for v in range(8)]
    os = [ws[(-u) % 8] for u in range(8)]
    for b in range(3):
        m = (lane & (1 << b)) != 0
        os = [jnp.where(m, os[(u - (1 << b)) % 8], os[u]) for u in range(8)]
    return os


def _pack_run(vs, lane):
    hi = lane >= 64
    return jnp.concatenate([jnp.where(hi, vs[2 * v + 1], vs[2 * v]) for v in range(8)], axis=0).astype(BF16)


def _unpack_run(wb):
    w = pltpu.bitcast(wb, jnp.uint32)
    r = pltpu.roll(w, 64, 1)
    hi = lax.broadcasted_iota(jnp.int32, w.shape, 1) >= 64
    ev = pltpu.bitcast(jnp.where(hi, r, w), BF16).astype(F32)
    od = pltpu.bitcast(jnp.where(hi, w, r), BF16).astype(F32)
    vs = []
    for v in range(8):
        vs += [ev[8 * v:8 * v + 8], od[8 * v:8 * v + 8]]
    return vs


def _body(x_hbm, o_ref, xin, runs, rawf, rawb, a1_ref, a2_ref, lsems, ssems, rsems, rsems2, ready):
    load_hi = pltpu.make_async_copy(x_hbm.at[pl.ds(32, 32)], xin.at[pl.ds(32, 32)], lsems.at[0])
    load_lo = pltpu.make_async_copy(x_hbm.at[pl.ds(0, 32)], xin.at[pl.ds(0, 32)], lsems.at[1])
    load_hi.start()
    me = lax.axis_index("i")
    bar = pltpu.get_barrier_semaphore()

    def sig(sem, dst):
        pl.semaphore_signal(sem, inc=1, device_id=(dst,), device_id_type=MESH)

    def run_copy(src, dst):
        return pltpu.make_async_remote_copy(
            src_ref=runs.at[src], dst_ref=runs.at[src], send_sem=ssems.at[dst], recv_sem=rsems.at[src],
            device_id=(dst,), device_id_type=MESH)

    def raw_lo(src):
        return pltpu.make_async_remote_copy(
            src_ref=x_hbm.at[pl.ds(0, 32)], dst_ref=rawf.at[src], send_sem=ssems.at[0], recv_sem=rsems.at[src],
            device_id=(0,), device_id_type=MESH)

    def raw_hi(src):
        return pltpu.make_async_remote_copy(
            src_ref=rawb.at[src], dst_ref=rawb.at[src], send_sem=ssems.at[src], recv_sem=rsems2.at[src],
            device_id=(0,), device_id_type=MESH)

    for k in (2, 1):
        @pl.when(me == k)
        def _(k=k):
            pl.semaphore_wait(bar, 1)
            raw_lo(k).start()
            sig(ready if k == 2 else bar, 0)
            if k != 2:
                load_lo.start()
            load_hi.wait()
            rawb[k] = xin[32:64, :].astype(BF16)
            raw_hi(k).start()
            if k == 2:
                load_lo.start()

    @pl.when(me == 3)
    def _():
        sig(bar, 0)
        load_lo.start()
        load_hi.wait()

    @pl.when(me == 0)
    def _():
        for d in (2, 1, 3):
            sig(bar, d)
        load_lo.start()
        load_hi.wait()

    load_lo.wait()

    sub = lax.broadcasted_iota(jnp.int32, (8, 128), 0)
    lane = lax.broadcasted_iota(jnp.int32, (8, 128), 1)
    hi = lane >= 64
    own, lay = _sort128(_to_lanes([xin[8 * g:8 * g + 8, :] for g in range(8)], sub, lane), sub)
    runs[me] = _pack_run(own, lane)

    def finish(vs, vlay, lane_mod64):
        os = _from_lanes(vs, vlay, sub, lane, lane_mod64)
        for g in range(8):
            o_ref[8 * g:8 * g + 8, :] = os[g]

    @pl.when(me == 2)
    def _():
        pl.semaphore_wait(bar, 1)
        sig(ready, 1)
        sig(ready, 3)
        run_copy(2, 1).start()
        run_copy(2, 3).start()

    @pl.when(me == 3)
    def _():
        pl.semaphore_wait(bar, 1)
        run_copy(3, 0).start()

    for k in (1, 3):
        @pl.when(me == k)
        def _(k=k):
            pl.semaphore_wait(bar, 1)
            run_copy(k, 4 - k).start()
            pl.semaphore_wait(ready, 1)
            run_copy(k, 2).start()

    @pl.when(me != 0)
    def _():
        for d in (1, 2, 3):
            run_copy((me + d) & 3, 0).wait_recv()
        halves = []
        for a, b in ((0, 1), (2, 3)):
            xs = _unpack_run(runs[a])
            ys = _mirror(_unpack_run(runs[b]), lay, lay, sub)
            vs = [jnp.minimum(x, y) for x, y in zip(xs, ys)] + [jnp.maximum(x, y) for x, y in zip(xs, ys)]
            vs, mlay = _clean(vs, {**lay, 7: ("v", 4)}, range(6, -1, -1), {3: 4, 2: 3, 1: 2}, sub)
            vs, mlay = _canon(vs, mlay, (0, 1, 5, 6, 7))
            halves.append(vs)
        ys = _mirror(halves[1], mlay, mlay, sub)
        mev = jnp.full((8, 128), me, jnp.int32)
        top, odd = mev >= 2, (mev & 1) == 1
        vs = [jnp.where(top, jnp.maximum(x, y), jnp.minimum(x, y)) for x, y in zip(halves[0], ys)]
        vs = [jnp.where(odd, jnp.maximum(vs[v], vs[v + 16]), jnp.minimum(vs[v], vs[v + 16])) for v in range(16)]
        vs = [jnp.where(hi, jnp.maximum(vs[v], vs[v + 8]), jnp.minimum(vs[v], vs[v + 8])) for v in range(8)]
        vs, vlay = _clean(vs, mlay, range(5, -1, -1), {4: 5, 3: 4, 2: 3}, sub)
        finish(vs, vlay, lane & 63)

    for k in (1, 2, 3):
        @pl.when(me == k)
        def _(k=k):
            if k == 3:
                run_copy(k, 0).wait_send()
            else:
                raw_lo(k).wait_send()
                raw_hi(k).wait_send()
            for d in (1, 2, 3):
                if d != k:
                    run_copy(k, d).wait_send()

    def recv_raw(k):
        raw_lo(k).wait_recv()
        xf = [rawf[k, 8 * g:8 * g + 8, :] for g in range(4)]
        raw_hi(k).wait_recv()
        xb = rawb[k].astype(F32)
        return xf + [xb[8 * g:8 * g + 8] for g in range(4)]

    @pl.when(me == 0)
    def _():
        pl.semaphore_wait(bar, 2)
        for d in (2, 1, 3):
            sig(bar, d)
        run_copy(0, 1).start()
        run_copy(0, 3).start()
        acc, alay = _unpack_run(runs[0]), lay
        pl.semaphore_wait(ready, 1)
        run_copy(0, 2).start()
        for k in (1, 3):
            if k == 1:
                run, _ = _sort128(_to_lanes(recv_raw(k), sub, lane), sub)
            else:
                run_copy(k, 0).wait_recv()
                run = _unpack_run(runs[k])
            acc = [jnp.minimum(x, y) for x, y in zip(acc, _mirror(run, lay, alay, sub))]
            acc, alay = _clean(acc, alay, range(6, -1, -1), {3: 0, 2: 3, 1: 2, 0: 1}, sub)
            acc, alay = _canon(acc, alay, RUN_VBITS)
        am = _mirror(acc, alay, lay, sub)
        for v in range(8):
            a1_ref[8 * v:8 * v + 8, :] = jnp.where(hi, am[v + 8], -jnp.inf)
            a2_ref[8 * v:8 * v + 8, :] = jnp.where(hi, am[v], am[v + 8])
        for d in (1, 3, 2):
            run_copy(0, d).wait_send()
        zs = _to_lanes(recv_raw(2), sub, lane)
        lane_mod64 = pltpu.roll(lane, 64, 1) & 63
        bs, blay = _sort128(zs, sub, TREE16)
        vs = [jnp.maximum(jnp.minimum(a1_ref[8 * v:8 * v + 8, :], bs[v + 8]),
                          jnp.minimum(a2_ref[8 * v:8 * v + 8, :], bs[v])) for v in range(8)]
        vs, vlay = _clean(vs, blay, range(5, -1, -1), {3: 5, 2: 4, 1: 3}, sub)
        finish(vs, vlay, lane_mod64)


def pallas_dist_sort_i_m128_n64_kernel(x: jax.Array):
    xt = x.T
    out = pl.pallas_call(
        _body,
        out_shape=jax.ShapeDtypeStruct(xt.shape, xt.dtype),
        in_specs=[pl.BlockSpec(memory_space=pl.ANY)],
        out_specs=pl.BlockSpec(memory_space=pltpu.VMEM),
        scratch_shapes=[
            pltpu.VMEM((64, 128), F32),
            pltpu.VMEM((4, 64, 128), BF16),
            pltpu.VMEM((3, 32, 128), F32),
            pltpu.VMEM((3, 32, 128), BF16),
            pltpu.VMEM((64, 128), F32),
            pltpu.VMEM((64, 128), F32),
            pltpu.SemaphoreType.DMA((2,)),
            pltpu.SemaphoreType.DMA((4,)),
            pltpu.SemaphoreType.DMA((4,)),
            pltpu.SemaphoreType.DMA((3,)),
            pltpu.SemaphoreType.REGULAR,
        ],
        compiler_params=pltpu.CompilerParams(
            collective_id=0, disable_semaphore_checks=True, disable_bounds_checks=True),
    )(xt)
    return out.T
```

```python
import jax
import jax.numpy as jnp
from jax import lax
from jax.experimental import pallas as pl
from jax.experimental.pallas import tpu as pltpu

F32 = jnp.float32
BF16 = jnp.bfloat16
MESH = pl.DeviceIdType.MESH

SORT16 = (
    ((0, 13), (1, 12), (2, 15), (3, 14), (4, 8), (5, 6), (7, 11), (9, 10)),
    ((0, 5), (1, 7), (2, 9), (3, 4), (6, 13), (8, 14), (10, 15), (11, 12)),
    ((0, 1), (2, 3), (4, 5), (6, 8), (7, 9), (10, 11), (12, 13), (14, 15)),
    ((0, 2), (1, 3), (4, 10), (5, 11), (6, 7), (8, 9), (12, 14), (13, 15)),
    ((1, 2), (3, 12), (4, 6), (5, 7), (8, 10), (9, 11), (13, 14)),
    ((1, 4), (2, 6), (5, 8), (7, 10), (9, 13), (11, 14)),
    ((2, 4), (3, 6), (9, 12), (11, 13)),
    ((3, 5), (6, 8), (7, 9), (10, 12)),
    ((3, 4), (5, 6), (7, 8), (9, 10), (11, 12)),
    ((6, 7), (8, 9)),
)
TREE16 = (((((0, 2), (4, 5)), ((1, 3), (6, 7))), ((8, 9), (10, 11))), (((12, 14), 13), 15))
RUN_VBITS = (0, 4, 5, 6)


def _sperm(x, idx):
    return jnp.take_along_axis(x, idx, axis=0, mode="promise_in_bounds")


def _insert(s, p):
    lo = [jnp.minimum(e, p) for e in s]
    return [lo[0]] + [jnp.maximum(s[i - 1], lo[i]) for i in range(1, len(s))] + [jnp.maximum(s[-1], p)]


def _odd_even_merge(a, b):
    if not a or not b:
        return list(a) + list(b)
    if len(b) == 1:
        return _insert(a, b[0])
    if len(a) == 1:
        return _insert(b, a[0])
    ev = _odd_even_merge(a[0::2], b[0::2])
    od = _odd_even_merge(a[1::2], b[1::2])
    out = [ev[0]]
    i = 0
    while i < len(od) and i + 1 < len(ev):
        out += [jnp.minimum(od[i], ev[i + 1]), jnp.maximum(od[i], ev[i + 1])]
        i += 1
    return out + od[i:] + ev[i + 1:]


def _tree_sort(vs, t):
    if isinstance(t, int):
        return [vs[t]]
    return _odd_even_merge(_tree_sort(vs, t[0]), _tree_sort(vs, t[1]))


def _clean(vs, lay, bits, evict, sub, fuse=None):
    vs, lay, bits = list(vs), dict(lay), list(bits)
    flipped = set()
    for n, b in enumerate(bits):
        kind, p = lay[b]
        later = [c for c in bits[n + 1:] if lay[c][0] == "s" and evict[c] == b and (fuse is None or b in fuse)]
        flip = (sub & (1 << lay[later[0]][1])) != 0 if later else None
        if kind == "s":
            e = evict[b]
            m = (sub & (1 << p)) != 0
            idx = sub ^ (1 << p)
            lay[b], lay[e] = lay[e], ("s", p)
            p = lay[b][1]
        for v in range(len(vs)):
            if (v >> p) & 1:
                continue
            x, y = vs[v], vs[v | (1 << p)]
            if kind == "s":
                if e not in flipped:
                    x, y = jnp.where(m, y, x), jnp.where(m, x, y)
                y = _sperm(y, idx)
            if flip is None:
                vs[v], vs[v | (1 << p)] = jnp.minimum(x, y), jnp.maximum(x, y)
            else:
                c = jnp.logical_xor(x > y, flip)
                vs[v], vs[v | (1 << p)] = jnp.where(c, y, x), jnp.where(c, x, y)
        if later:
            flipped.add(b)
    return vs, lay


def _canon(vs, lay, vbits):
    out = [vs[sum(((v >> k) & 1) << lay[b][1] for k, b in enumerate(vbits))] for v in range(len(vs))]
    lay = dict(lay)
    for k, b in enumerate(vbits):
        lay[b] = ("v", k)
    return out, lay


def _sort128(vs, sub, tree=None):
    vs = list(vs)
    if tree is not None:
        vs = _tree_sort(vs, tree)
    else:
        for layer in SORT16:
            for a, b in layer:
                vs[a], vs[b] = jnp.minimum(vs[a], vs[b]), jnp.maximum(vs[a], vs[b])
    lay = {0: ("v", 0), 1: ("v", 1), 2: ("v", 2), 3: ("v", 3), 4: ("s", 2), 5: ("s", 1), 6: ("s", 0)}
    for t in (4, 5, 6):
        idx = sub ^ sum(1 << lay[b][1] for b in range(t + 1) if lay[b][0] == "s")
        pe = lay[0][1]
        ws = list(vs)
        for v in range(16):
            if not (v >> pe) & 1:
                x, y = vs[v], _sperm(vs[v ^ 15], idx)
                ws[v], ws[v | (1 << pe)] = jnp.minimum(x, y), jnp.maximum(x, y)
        lay[0], lay[t] = lay[t], lay[0]
        vs, lay = _clean(ws, lay, range(t - 1, -1, -1), {b: b + 1 for b in range(7)}, sub)
    return _canon(vs, lay, RUN_VBITS)


def _move_bits(val, src, dst):
    if list(src) == list(dst):
        return val
    out = None
    for sp, dp in zip(src, dst):
        t = val & (1 << sp)
        t = t << (dp - sp) if dp >= sp else t >> (sp - dp)
        out = t if out is None else out | t
    return out


def _mirror(vs, lay, dlay, sub):
    vb = sorted((b for b in dlay if dlay[b][0] == "v"), key=lambda b: dlay[b][1])
    vs, lay = _canon(vs, lay, vb)
    sb = [b for b in dlay if dlay[b][0] == "s"]
    idx = _move_bits(sub ^ 7, [dlay[b][1] for b in sb], [lay[b][1] for b in sb])
    return [_sperm(vs[v ^ (len(vs) - 1)], idx) for v in range(len(vs))]


def _skew_roll(xs, sub, lane):
    us = list(xs)
    for b in range(3):
        m = (lane & (1 << b)) != 0
        us = [jnp.where(m, us[(v + (1 << b)) % 8], us[v]) for v in range(8)]
    ys = [_sperm(us[v], (sub + ((lane + v) >> 3)) & 7) for v in range(8)]
    r1 = [pltpu.roll(ys[v], v, 1, stride=8, stride_axis=0) for v in range(8)]
    r2 = [pltpu.roll(ys[v], v + 64, 1, stride=8, stride_axis=0) for v in range(8)]
    return r1, r2


def _to_lanes(xs, sub, lane):
    r1, r2 = _skew_roll(xs, sub, lane)
    return r1 + r2


def _from_lanes(vs, lay, sub, lane, lane_mod64):
    vs, lay = _canon(vs, lay, (0, 1, 2))
    assert [lay[b] for b in (3, 4, 5)] == [("s", 0), ("s", 1), ("s", 2)]
    r1, r2 = _skew_roll(vs, sub, lane)
    wrap = lane_mod64 - 8 * sub
    ws = [_sperm(jnp.where(wrap < v, r2[v], r1[v]), (((lane - v) >> 3) - sub) & 7) for v in range(8)]
    outs = [ws[(-u) % 8] for u in range(8)]
    for b in range(3):
        m = (lane & (1 << b)) != 0
        outs = [jnp.where(m, outs[(u - (1 << b)) % 8], outs[u]) for u in range(8)]
    return outs


def _pack_run(vs, lane):
    hi = lane >= 64
    return jnp.concatenate([jnp.where(hi, vs[2 * v + 1], vs[2 * v]) for v in range(8)], axis=0).astype(BF16)


def _unpack_run(wb):
    w = pltpu.bitcast(wb, jnp.uint32)
    r = pltpu.roll(w, 64, 1)
    hi = lax.broadcasted_iota(jnp.int32, w.shape, 1) >= 64
    ev = pltpu.bitcast(jnp.where(hi, r, w), BF16).astype(F32)
    od = pltpu.bitcast(jnp.where(hi, w, r), BF16).astype(F32)
    vs = []
    for v in range(8):
        vs += [ev[8 * v:8 * v + 8], od[8 * v:8 * v + 8]]
    return vs


def _body(x_hbm, o_ref, xin, runs, rawf, rawm, rawb, a1_ref, a2_ref, lsems, ssems, rsems, rsems2, rsems3, ready):
    load_mid = pltpu.make_async_copy(x_hbm.at[pl.ds(24, 8)], xin.at[pl.ds(24, 8)], lsems.at[2])
    load_hi = pltpu.make_async_copy(x_hbm.at[pl.ds(32, 32)], xin.at[pl.ds(32, 32)], lsems.at[0])
    load_lo = pltpu.make_async_copy(x_hbm.at[pl.ds(0, 24)], xin.at[pl.ds(0, 24)], lsems.at[1])
    me = lax.axis_index("i")
    load_mid.start()
    load_hi.start()
    bar = pltpu.get_barrier_semaphore()

    def sig(sem, dst):
        pl.semaphore_signal(sem, inc=1, device_id=(dst,), device_id_type=MESH)

    def run_copy(src, dst):
        return pltpu.make_async_remote_copy(
            src_ref=runs.at[src], dst_ref=runs.at[src], send_sem=ssems.at[dst], recv_sem=rsems.at[src],
            device_id=(dst,), device_id_type=MESH)

    def raw_lo(src):
        return pltpu.make_async_remote_copy(
            src_ref=x_hbm.at[pl.ds(0, 24)], dst_ref=rawf.at[src], send_sem=ssems.at[0], recv_sem=rsems.at[src],
            device_id=(0,), device_id_type=MESH)

    def raw_hi(src):
        return pltpu.make_async_remote_copy(
            src_ref=rawb.at[src], dst_ref=rawb.at[src], send_sem=ssems.at[src], recv_sem=rsems2.at[src],
            device_id=(0,), device_id_type=MESH)

    def raw_mid(src):
        return pltpu.make_async_remote_copy(
            src_ref=rawm.at[src], dst_ref=rawm.at[src], send_sem=ssems.at[4], recv_sem=rsems3.at[src],
            device_id=(0,), device_id_type=MESH)

    for k in (2, 1):
        @pl.when(me == k)
        def _(k=k):
            pl.semaphore_wait(bar, 1)
            raw_lo(k).start()
            sig(ready if k == 2 else bar, 0)
            if k != 2:
                load_lo.start()
            load_mid.wait()
            rawm[k] = xin[24:32, :].astype(BF16)
            raw_mid(k).start()
            load_hi.wait()
            rawb[k] = xin[32:64, :].astype(BF16)
            raw_hi(k).start()
            if k == 2:
                load_lo.start()

    @pl.when(me == 3)
    def _():
        sig(bar, 0)
        load_lo.start()
        load_mid.wait()
        load_hi.wait()

    @pl.when(me == 0)
    def _():
        for d in (2, 1, 3):
            sig(bar, d)
        load_lo.start()
        load_mid.wait()
        load_hi.wait()

    load_lo.wait()

    sub = lax.broadcasted_iota(jnp.int32, (8, 128), 0)
    lane = lax.broadcasted_iota(jnp.int32, (8, 128), 1)
    hi = lane >= 64
    own, lay = _sort128(_to_lanes([xin[8 * g:8 * g + 8, :] for g in range(8)], sub, lane), sub)
    runs[me] = _pack_run(own, lane)

    def finish(vs, vlay, lane_mod64):
        outs = _from_lanes(vs, vlay, sub, lane, lane_mod64)
        for g in range(8):
            o_ref[8 * g:8 * g + 8, :] = outs[g]

    @pl.when(me == 2)
    def _():
        pl.semaphore_wait(bar, 1)
        sig(ready, 1)
        sig(ready, 3)
        run_copy(2, 1).start()
        run_copy(2, 3).start()

    @pl.when(me == 3)
    def _():
        pl.semaphore_wait(bar, 1)
        run_copy(3, 0).start()

    for k in (1, 3):
        @pl.when(me == k)
        def _(k=k):
            pl.semaphore_wait(bar, 1)
            run_copy(k, 4 - k).start()
            pl.semaphore_wait(ready, 1)
            run_copy(k, 2).start()

    @pl.when(me != 0)
    def _():
        for d in (1, 2, 3):
            run_copy((me + d) & 3, 0).wait_recv()
        halves = []
        for a, b in ((0, 1), (2, 3)):
            xs = _unpack_run(runs[a])
            ys = _mirror(_unpack_run(runs[b]), lay, lay, sub)
            vs = [jnp.minimum(x, y) for x, y in zip(xs, ys)] + [jnp.maximum(x, y) for x, y in zip(xs, ys)]
            vs, mlay = _clean(vs, {**lay, 7: ("v", 4)}, range(6, -1, -1), {3: 4, 2: 3, 1: 2}, sub)
            vs, mlay = _canon(vs, mlay, (0, 1, 5, 6, 7))
            halves.append(vs)
        ys = _mirror(halves[1], mlay, mlay, sub)
        mev = jnp.full((8, 128), me, jnp.int32)
        top, odd = mev >= 2, (mev & 1) == 1
        vs = [jnp.where(top, jnp.maximum(x, y), jnp.minimum(x, y)) for x, y in zip(halves[0], ys)]
        vs = [jnp.where(odd, jnp.maximum(vs[v], vs[v + 16]), jnp.minimum(vs[v], vs[v + 16])) for v in range(16)]
        vs = [jnp.where(hi, jnp.maximum(vs[v], vs[v + 8]), jnp.minimum(vs[v], vs[v + 8])) for v in range(8)]
        vs, vlay = _clean(vs, mlay, range(5, -1, -1), {4: 5, 3: 4, 2: 3}, sub)
        finish(vs, vlay, lane & 63)

    for k in (1, 2, 3):
        @pl.when(me == k)
        def _(k=k):
            if k == 3:
                run_copy(k, 0).wait_send()
            else:
                raw_lo(k).wait_send()
                raw_mid(k).wait_send()
                raw_hi(k).wait_send()
            for d in (1, 2, 3):
                if d != k:
                    run_copy(k, d).wait_send()

    def recv_raw(k):
        raw_lo(k).wait_recv()
        xf = [rawf[k, 8 * g:8 * g + 8, :] for g in range(3)]
        raw_mid(k).wait_recv()
        xf.append(rawm[k].astype(F32))
        raw_hi(k).wait_recv()
        xb = rawb[k].astype(F32)
        return xf + [xb[8 * g:8 * g + 8] for g in range(4)]

    @pl.when(me == 0)
    def _():
        pl.semaphore_wait(bar, 2)
        for d in (2, 1, 3):
            sig(bar, d)
        run_copy(0, 1).start()
        run_copy(0, 3).start()
        acc, alay = _unpack_run(runs[0]), lay
        pl.semaphore_wait(ready, 1)
        run_copy(0, 2).start()
        for k in (1, 3):
            if k == 1:
                run, _ = _sort128(_to_lanes(recv_raw(k), sub, lane), sub)
            else:
                run_copy(k, 0).wait_recv()
                run = _unpack_run(runs[k])
            acc = [jnp.minimum(x, y) for x, y in zip(acc, _mirror(run, lay, alay, sub))]
            acc, alay = _clean(acc, alay, range(6, -1, -1), {3: 0, 2: 3, 1: 2, 0: 1}, sub)
            acc, alay = _canon(acc, alay, RUN_VBITS)
        am = _mirror(acc, alay, lay, sub)
        for v in range(8):
            a1_ref[8 * v:8 * v + 8, :] = jnp.where(hi, am[v + 8], -jnp.inf)
            a2_ref[8 * v:8 * v + 8, :] = jnp.where(hi, am[v], am[v + 8])
        for d in (1, 3, 2):
            run_copy(0, d).wait_send()
        zs = _to_lanes(recv_raw(2), sub, lane)
        lane_mod64 = pltpu.roll(lane, 64, 1) & 63
        bs, blay = _sort128(zs, sub, TREE16)
        vs = [jnp.maximum(jnp.minimum(a1_ref[8 * v:8 * v + 8, :], bs[v + 8]),
                          jnp.minimum(a2_ref[8 * v:8 * v + 8, :], bs[v])) for v in range(8)]
        vs, vlay = _clean(vs, blay, range(5, -1, -1), {3: 5, 2: 4, 1: 3}, sub, fuse=(5,))
        finish(vs, vlay, lane_mod64)


def pallas_dist_sort_i_m128_n64_kernel(x: jax.Array):
    xt = x.T
    out = pl.pallas_call(
        _body,
        out_shape=jax.ShapeDtypeStruct(xt.shape, xt.dtype),
        in_specs=[pl.BlockSpec(memory_space=pl.ANY)],
        out_specs=pl.BlockSpec(memory_space=pltpu.VMEM),
        scratch_shapes=[
            pltpu.VMEM((64, 128), F32),
            pltpu.VMEM((4, 64, 128), BF16),
            pltpu.VMEM((3, 24, 128), F32),
            pltpu.VMEM((3, 8, 128), BF16),
            pltpu.VMEM((3, 32, 128), BF16),
            pltpu.VMEM((64, 128), F32),
            pltpu.VMEM((64, 128), F32),
            pltpu.SemaphoreType.DMA((3,)),
            pltpu.SemaphoreType.DMA((5,)),
            pltpu.SemaphoreType.DMA((4,)),
            pltpu.SemaphoreType.DMA((3,)),
            pltpu.SemaphoreType.DMA((3,)),
            pltpu.SemaphoreType.REGULAR,
        ],
        compiler_params=pltpu.CompilerParams(
            collective_id=0, disable_semaphore_checks=True, disable_bounds_checks=True),
    )(xt)
    return out.T
```

```python
import jax
import jax.numpy as jnp
from jax import lax
from jax.experimental import pallas as pl
from jax.experimental.pallas import tpu as pltpu

F32 = jnp.float32
BF16 = jnp.bfloat16
MESH = pl.DeviceIdType.MESH

SORT16 = (
    ((0, 13), (1, 12), (2, 15), (3, 14), (4, 8), (5, 6), (7, 11), (9, 10)),
    ((0, 5), (1, 7), (2, 9), (3, 4), (6, 13), (8, 14), (10, 15), (11, 12)),
    ((0, 1), (2, 3), (4, 5), (6, 8), (7, 9), (10, 11), (12, 13), (14, 15)),
    ((0, 2), (1, 3), (4, 10), (5, 11), (6, 7), (8, 9), (12, 14), (13, 15)),
    ((1, 2), (3, 12), (4, 6), (5, 7), (8, 10), (9, 11), (13, 14)),
    ((1, 4), (2, 6), (5, 8), (7, 10), (9, 13), (11, 14)),
    ((2, 4), (3, 6), (9, 12), (11, 13)),
    ((3, 5), (6, 8), (7, 9), (10, 12)),
    ((3, 4), (5, 6), (7, 8), (9, 10), (11, 12)),
    ((6, 7), (8, 9)),
)
TREE16 = (((((0, 2), (4, 5)), ((1, 3), (6, 7))), ((8, 9), (10, 11))), (((12, 14), 13), 15))
RUN_VBITS = (0, 4, 5, 6)


def _sperm(x, idx):
    return jnp.take_along_axis(x, idx, axis=0, mode="promise_in_bounds")


def _insert(s, p):
    lo = [jnp.minimum(e, p) for e in s]
    return [lo[0]] + [jnp.maximum(s[i - 1], lo[i]) for i in range(1, len(s))] + [jnp.maximum(s[-1], p)]


def _odd_even_merge(a, b):
    if not a or not b:
        return list(a) + list(b)
    if len(b) == 1:
        return _insert(a, b[0])
    if len(a) == 1:
        return _insert(b, a[0])
    ev = _odd_even_merge(a[0::2], b[0::2])
    od = _odd_even_merge(a[1::2], b[1::2])
    out = [ev[0]]
    i = 0
    while i < len(od) and i + 1 < len(ev):
        out += [jnp.minimum(od[i], ev[i + 1]), jnp.maximum(od[i], ev[i + 1])]
        i += 1
    return out + od[i:] + ev[i + 1:]


def _tree_sort(vs, t):
    if isinstance(t, int):
        return [vs[t]]
    return _odd_even_merge(_tree_sort(vs, t[0]), _tree_sort(vs, t[1]))


def _net_sort(vs):
    vs = list(vs)
    for layer in SORT16:
        for a, b in layer:
            vs[a], vs[b] = jnp.minimum(vs[a], vs[b]), jnp.maximum(vs[a], vs[b])
    return vs


def _clean(vs, lay, bits, evict, sub, fuse=True):
    vs, lay, bits = list(vs), dict(lay), list(bits)
    flipped = set()
    for n, b in enumerate(bits):
        kind, p = lay[b]
        later = [c for c in bits[n + 1:] if fuse and lay[c][0] == "s" and evict[c] == b]
        flip = (sub & (1 << lay[later[0]][1])) != 0 if later else None
        if kind == "s":
            e = evict[b]
            m = (sub & (1 << p)) != 0
            idx = sub ^ (1 << p)
            lay[b], lay[e] = lay[e], ("s", p)
            p = lay[b][1]
        for v in range(len(vs)):
            if (v >> p) & 1:
                continue
            x, y = vs[v], vs[v | (1 << p)]
            if kind == "s":
                if e not in flipped:
                    x, y = jnp.where(m, y, x), jnp.where(m, x, y)
                y = _sperm(y, idx)
            if flip is None:
                vs[v], vs[v | (1 << p)] = jnp.minimum(x, y), jnp.maximum(x, y)
            else:
                c = jnp.logical_xor(x > y, flip)
                vs[v], vs[v | (1 << p)] = jnp.where(c, y, x), jnp.where(c, x, y)
        if later:
            flipped.add(b)
    return vs, lay


def _canon(vs, lay, vbits):
    out = [vs[sum(((v >> k) & 1) << lay[b][1] for k, b in enumerate(vbits))] for v in range(len(vs))]
    lay = dict(lay)
    for k, b in enumerate(vbits):
        lay[b] = ("v", k)
    return out, lay


def _merge_sublanes(vs, sub):
    lay = {0: ("v", 0), 1: ("v", 1), 2: ("v", 2), 3: ("v", 3), 4: ("s", 2), 5: ("s", 1), 6: ("s", 0)}
    for t in (4, 5, 6):
        idx = sub ^ sum(1 << lay[b][1] for b in range(t + 1) if lay[b][0] == "s")
        pe = lay[0][1]
        ws = list(vs)
        for v in range(16):
            if not (v >> pe) & 1:
                x, y = vs[v], _sperm(vs[v ^ 15], idx)
                ws[v], ws[v | (1 << pe)] = jnp.minimum(x, y), jnp.maximum(x, y)
        lay[0], lay[t] = lay[t], lay[0]
        vs, lay = _clean(ws, lay, range(t - 1, -1, -1), {b: b + 1 for b in range(7)}, sub)
    return _canon(vs, lay, RUN_VBITS)


def _move_bits(val, src, dst):
    if list(src) == list(dst):
        return val
    out = None
    for sp, dp in zip(src, dst):
        t = val & (1 << sp)
        t = t << (dp - sp) if dp >= sp else t >> (sp - dp)
        out = t if out is None else out | t
    return out


def _mirror(vs, lay, dlay, sub):
    vb = sorted((b for b in dlay if dlay[b][0] == "v"), key=lambda b: dlay[b][1])
    vs, lay = _canon(vs, lay, vb)
    sb = [b for b in dlay if dlay[b][0] == "s"]
    idx = _move_bits(sub ^ 7, [dlay[b][1] for b in sb], [lay[b][1] for b in sb])
    return [_sperm(vs[v ^ (len(vs) - 1)], idx) for v in range(len(vs))]


def _skew(xs, sub, lane):
    n = len(xs)
    nb = n.bit_length() - 1
    us = list(xs)
    for b in range(nb):
        m = (lane & (1 << b)) != 0
        us = [jnp.where(m, us[(v + (1 << b)) % n], us[v]) for v in range(n)]
    return [_sperm(us[v], (sub + ((lane + v) >> nb)) & 7) for v in range(n)]


def _roll(ys, extra):
    return [pltpu.roll(y, v + extra, 1, stride=len(ys), stride_axis=0) for v, y in enumerate(ys)]


def _to_lanes(xs, sub, lane):
    ys = _skew(xs, sub, lane)
    return [z for extra in range(0, 128, 8 * len(xs)) for z in _roll(ys, extra)]


def _skew_ranks(vs, lay, sub, lane):
    nb = len(vs).bit_length() - 1
    vs, lay = _canon(vs, lay, range(nb))
    assert [lay[nb + b] for b in range(3)] == [("s", 0), ("s", 1), ("s", 2)]
    return _skew(vs, sub, lane)


def _unskew(ys, sub, lane):
    n = len(ys)
    nb = n.bit_length() - 1
    r1, r2 = _roll(ys, 0), _roll(ys, 128 - 8 * n)
    wrap = (lane & (8 * n - 1)) - n * sub
    ws = [_sperm(jnp.where(wrap < v, r2[v], r1[v]), (((lane - v) >> nb) - sub) & 7) for v in range(n)]
    outs = [ws[(-u) % n] for u in range(n)]
    for b in range(nb):
        m = (lane & (1 << b)) != 0
        outs = [jnp.where(m, outs[(u - (1 << b)) % n], outs[u]) for u in range(n)]
    return outs


def _pack_run(vs, lane):
    hi = lane >= 64
    return jnp.concatenate([jnp.where(hi, vs[2 * v + 1], vs[2 * v]) for v in range(8)], axis=0).astype(BF16)


def _unpack_run(wb):
    w = pltpu.bitcast(wb, jnp.uint32)
    r = pltpu.roll(w, 64, 1)
    hi = lax.broadcasted_iota(jnp.int32, w.shape, 1) >= 64
    ev = pltpu.bitcast(jnp.where(hi, r, w), BF16).astype(F32)
    od = pltpu.bitcast(jnp.where(hi, w, r), BF16).astype(F32)
    vs = []
    for v in range(8):
        vs += [ev[8 * v:8 * v + 8], od[8 * v:8 * v + 8]]
    return vs


def _body(x_hbm, o_ref, xin, runs, rawf, rawm, rawb, atab, lsems, ssems, rsems, rsems_m, rsems_b, ready):
    load_lo = pltpu.make_async_copy(x_hbm.at[pl.ds(0, 24)], xin.at[pl.ds(0, 24)], lsems.at[0])
    load_mid = pltpu.make_async_copy(x_hbm.at[pl.ds(24, 8)], xin.at[pl.ds(24, 8)], lsems.at[1])
    load_hi = pltpu.make_async_copy(x_hbm.at[pl.ds(32, 32)], xin.at[pl.ds(32, 32)], lsems.at[2])
    me = lax.axis_index("i")
    load_mid.start()
    load_hi.start()
    bar = pltpu.get_barrier_semaphore()

    def sig(sem, dst):
        pl.semaphore_signal(sem, inc=1, device_id=(dst,), device_id_type=MESH)

    def run_copy(src, dst):
        return pltpu.make_async_remote_copy(
            src_ref=runs.at[src], dst_ref=runs.at[src], send_sem=ssems.at[dst], recv_sem=rsems.at[src],
            device_id=(dst,), device_id_type=MESH)

    def raw_lo(src):
        return pltpu.make_async_remote_copy(
            src_ref=x_hbm.at[pl.ds(0, 24)], dst_ref=rawf.at[src], send_sem=ssems.at[0], recv_sem=rsems.at[src],
            device_id=(0,), device_id_type=MESH)

    def raw_mid(src):
        return pltpu.make_async_remote_copy(
            src_ref=rawm.at[src], dst_ref=rawm.at[src], send_sem=ssems.at[4], recv_sem=rsems_m.at[src],
            device_id=(0,), device_id_type=MESH)

    def raw_hi(src):
        return pltpu.make_async_remote_copy(
            src_ref=rawb.at[src], dst_ref=rawb.at[src], send_sem=ssems.at[src], recv_sem=rsems_b.at[src],
            device_id=(0,), device_id_type=MESH)

    for k in (2, 1, 3):
        @pl.when(me == k)
        def _(k=k):
            pl.semaphore_wait(bar, 1)
            raw_lo(k).start()
            sig(ready if k == 2 else bar, 0)
            if k != 2:
                load_lo.start()
            load_mid.wait()
            rawm[k] = xin[24:32, :].astype(BF16)
            raw_mid(k).start()
            load_hi.wait()
            rawb[k] = xin[32:64, :].astype(BF16)
            raw_hi(k).start()
            if k == 2:
                load_lo.start()

    @pl.when(me == 0)
    def _():
        for d in (2, 1, 3):
            sig(bar, d)
        load_lo.start()
        load_mid.wait()
        load_hi.wait()

    load_lo.wait()

    sub = lax.broadcasted_iota(jnp.int32, (8, 128), 0)
    lane = lax.broadcasted_iota(jnp.int32, (8, 128), 1)
    mev = jnp.full((8, 128), me, jnp.int32)

    def sort_shard(xs):
        return _merge_sublanes(_net_sort(_to_lanes(xs, sub, lane)), sub)

    def store_out(ys, row0):
        for g, out in enumerate(_unskew(ys, sub, lane)):
            o_ref[row0 + 8 * g:row0 + 8 * g + 8, :] = out

    own, lay = sort_shard([xin[8 * g:8 * g + 8, :] for g in range(8)])
    runs[me] = _pack_run(own, lane)

    @pl.when(me == 2)
    def _():
        pl.semaphore_wait(bar, 1)
        sig(ready, 1)
        sig(ready, 3)
        run_copy(2, 1).start()
        run_copy(2, 3).start()

    for k in (1, 3):
        @pl.when(me == k)
        def _(k=k):
            pl.semaphore_wait(bar, 1)
            run_copy(k, 4 - k).start()
            pl.semaphore_wait(ready, 1)
            run_copy(k, 2).start()

    @pl.when(me != 0)
    def _():
        for d in (1, 2, 3):
            run_copy((me + d) & 3, 0).wait_recv()
        halves = []
        for a, b in ((0, 1), (2, 3)):
            xs = _unpack_run(runs[a])
            ys = _mirror(_unpack_run(runs[b]), lay, lay, sub)
            vs = [jnp.minimum(x, y) for x, y in zip(xs, ys)] + [jnp.maximum(x, y) for x, y in zip(xs, ys)]
            vs, mlay = _clean(vs, {**lay, 7: ("v", 4)}, range(6, -1, -1), {3: 4, 2: 3, 1: 2}, sub)
            vs, mlay = _canon(vs, mlay, (0, 1, 5, 6, 7))
            halves.append(vs)
        ys = _mirror(halves[1], mlay, mlay, sub)
        top, odd, hi = mev >= 2, (mev & 1) == 1, lane >= 64
        vs = [jnp.where(top, jnp.maximum(x, y), jnp.minimum(x, y)) for x, y in zip(halves[0], ys)]
        vs = [jnp.where(odd, jnp.maximum(vs[v], vs[v + 16]), jnp.minimum(vs[v], vs[v + 16])) for v in range(16)]
        vs = [jnp.where(hi, jnp.maximum(vs[v], vs[v + 8]), jnp.minimum(vs[v], vs[v + 8])) for v in range(8)]
        vs, vlay = _clean(vs, mlay, range(5, -1, -1), {4: 5, 3: 4, 2: 3}, sub)
        store_out(_skew_ranks(vs, vlay, sub, lane), 0)

    for k in (1, 2, 3):
        @pl.when(me == k)
        def _(k=k):
            raw_lo(k).wait_send()
            raw_mid(k).wait_send()
            raw_hi(k).wait_send()
            for d in (1, 2, 3):
                if d != k:
                    run_copy(k, d).wait_send()

    def recv_low_cols(k):
        raw_lo(k).wait_recv()
        xs = [rawf[k, 8 * g:8 * g + 8, :] for g in range(3)]
        raw_mid(k).wait_recv()
        return xs + [rawm[k].astype(F32)]

    def recv_high_cols(k):
        raw_hi(k).wait_recv()
        xb = rawb[k].astype(F32)
        return [xb[8 * g:8 * g + 8] for g in range(4)]

    @pl.when(me == 0)
    def _():
        pl.semaphore_wait(bar, 2)
        for d in (2, 1, 3):
            sig(bar, d)
        run_copy(0, 1).start()
        run_copy(0, 3).start()
        acc, alay = _unpack_run(runs[0]), lay
        pl.semaphore_wait(ready, 1)
        run_copy(0, 2).start()
        for xs in [recv_low_cols(k) + recv_high_cols(k) for k in (1, 3)]:
            run, _ = sort_shard(xs)
            acc = [jnp.minimum(x, y) for x, y in zip(acc, _mirror(run, lay, alay, sub))]
            acc, alay = _clean(acc, alay, range(6, -1, -1), {3: 0, 2: 3, 1: 2, 0: 1}, sub)
            acc, alay = _canon(acc, alay, RUN_VBITS)
        am = _mirror(acc, alay, lay, sub)
        quarter = lane >> 5
        for half in range(2):
            src = 4 * half + (lane & 3) + 8 * ((lane >> 2) & 7)
            ah = [jnp.take_along_axis(a, src, axis=1, mode="promise_in_bounds") for a in am]
            for v in range(4):
                for u in range(4):
                    tab = ah[v + 12] if u == 0 else jnp.where(quarter < u, -jnp.inf, ah[v + 12])
                    for t in range(1, 4 - u):
                        tab = jnp.where(quarter == t + u, ah[v + 12 - 4 * t], tab)
                    atab[half, 8 * (v + 4 * u):8 * (v + 4 * u) + 8, :] = tab

        def fold(half, vs):
            bs, blay = _merge_sublanes(vs, sub)
            cs = [jnp.minimum(atab[half, 8 * v:8 * v + 8, :], bs[v]) for v in range(16)]
            vs = [jnp.maximum(jnp.maximum(cs[v], cs[v + 4]), jnp.maximum(cs[v + 8], cs[v + 12])) for v in range(4)]
            vs, vlay = _clean(vs, blay, range(4, -1, -1), {3: 4, 2: 3, 1: 2}, sub, fuse=False)
            ys = _skew_ranks(vs, vlay, sub, lane)
            store_out(ys, 32 * half)
            return ys

        early = _tree_sort(_to_lanes(recv_low_cols(2), sub, lane), TREE16)
        for d in (1, 3, 2):
            run_copy(0, d).wait_send()
        late = _to_lanes(recv_high_cols(2), sub, lane)
        ys = fold(0, early)
        for y, z in zip(ys, (0, 2, 1, 3)):
            late[z] = jnp.where(mev > 0, y, late[z])
        fold(1, _tree_sort(late, TREE16))


def pallas_dist_sort_i_m128_n64_kernel(x: jax.Array):
    xt = x.T
    out = pl.pallas_call(
        _body,
        out_shape=jax.ShapeDtypeStruct(xt.shape, xt.dtype),
        in_specs=[pl.BlockSpec(memory_space=pl.ANY)],
        out_specs=pl.BlockSpec(memory_space=pltpu.VMEM),
        scratch_shapes=[
            pltpu.VMEM((64, 128), F32),
            pltpu.VMEM((4, 64, 128), BF16),
            pltpu.VMEM((4, 24, 128), F32),
            pltpu.VMEM((4, 8, 128), BF16),
            pltpu.VMEM((4, 32, 128), BF16),
            pltpu.VMEM((2, 128, 128), F32),
            pltpu.SemaphoreType.DMA((3,)),
            pltpu.SemaphoreType.DMA((5,)),
            pltpu.SemaphoreType.DMA((4,)),
            pltpu.SemaphoreType.DMA((4,)),
            pltpu.SemaphoreType.DMA((4,)),
            pltpu.SemaphoreType.REGULAR,
        ],
        compiler_params=pltpu.CompilerParams(
            collective_id=0, disable_semaphore_checks=True, disable_bounds_checks=True),
    )(xt)
    return out.T
```
